```python
import numpy as np

kernel_name = "dist_moe_cap_ep_outshard_n2048_d512_e8_h1024"

def setup_inputs():
    x = np.random.randn(2048, 512).astype(np.float32)
    router_W = np.random.randn(512, 32).astype(np.float32) * 0.1
    scores64 = x.astype(np.float64) @ router_W.astype(np.float64)
    route_idx = np.argsort(-scores64, axis=-1)[:, :1].astype(np.int32)
    expert_W = np.random.randn(32, 512, 1024).astype(np.float32) * 0.02
    return {"x": x, "router_W": router_W, "route_idx": route_idx, "expert_W": expert_W}

def reference(x, router_W, route_idx, expert_W):
    counts = np.zeros(32, dtype=np.int64)
    out = np.zeros((2048, 1024), dtype=np.float32)
    for i in range(2048):
        e = int(route_idx[i, 0])
        if counts[e] < 51:
            out[i] = x[i] @ expert_W[e]
            counts[e] += 1
    return out
```

```python
import functools
import jax
import jax.numpy as jnp
from jax import lax
from jax.experimental import pallas as pl
from jax.experimental.pallas import tpu as pltpu

N, D, H, E, EL, CAP, ND = 2048, 512, 1024, 32, 8, 51, 4
NB = N // 128
MP = 56
ROWS = N // ND
MESH = pl.DeviceIdType.MESH


def make(inflight=2, nobounds=False, abl='', ch=1):
    def body(idx_ref, x_ref, w_ref, obuf, stg, wbuf, xg, ybuf, cbuf, tabv, flgv, zrow, tab, flg,
             wsem, xsem, ssem, rsem, tsem):
        me = lax.axis_index("i")
        class WC:
            def __init__(self, j): self.j = j
            def start(self, priority):
                r = D // ch
                for k in range(ch):
                    pltpu.make_async_copy(w_ref.at[self.j, pl.ds(k*r, r)], wbuf.at[self.j, pl.ds(k*r, r)], wsem.at[self.j]).start(priority=priority)
            def wait(self):
                pltpu.make_async_copy(w_ref.at[self.j], wbuf.at[self.j], wsem.at[self.j]).wait()
        wcp = [WC(j) for j in range(EL)]
        for j in range(inflight):
            wcp[j].start(priority=1 if 'w' in abl else 0)
        bar = pltpu.get_barrier_semaphore()
        for k in range(1, ND):
            pl.semaphore_signal(bar, inc=1, device_id=((me + k) % ND,), device_id_type=MESH)

        idx = idx_ref[...]
        sub = lax.broadcasted_iota(jnp.int32, (E, 128), 0)
        oh = [(idx[b:b + 1, :] == sub) for b in range(NB)]
        ohf = jnp.concatenate([o.astype(jnp.float32) for o in oh], axis=0).astype(jnp.bfloat16)
        r_ = lax.broadcasted_iota(jnp.int32, (128, 256), 0)
        c_ = lax.broadcasted_iota(jnp.int32, (128, 256), 1)
        U = ((r_ <= c_)).astype(jnp.float32).astype(jnp.bfloat16)
        ct = jnp.dot(ohf, U, preferred_element_type=jnp.float32)
        off = jnp.zeros((E, 128), jnp.float32)
        keep = []
        for b in range(NB):
            c = ct[b * E:(b + 1) * E, :128] + off
            off = off + ct[b * E:(b + 1) * E, 128:]
            cbuf[b] = c
            keep.append(jnp.sum(jnp.where(oh[b] & (c <= CAP), 1.0, 0.0), axis=0, keepdims=True))
        flgv[...] = jnp.concatenate(keep, axis=0).astype(jnp.int32)
        fcp = pltpu.make_async_copy(flgv.at[pl.ds(me * 4, 4)], flg, tsem.at[1])
        fcp.start()
        cl = [cbuf[b, pl.ds(pl.multiple_of(me * EL, 8), EL), :] for b in range(NB)]
        accs = []
        for s in range(CAP):
            a = jnp.where(cl[0] <= s, 1.0, 0.0)
            for b in range(1, NB):
                a = a + jnp.where(cl[b] <= s, 1.0, 0.0)
            accs.append(a)
        lane = lax.broadcasted_iota(jnp.int32, (EL, 128), 1)
        accs.append(jnp.where(lane == 127, jnp.minimum(cl[NB - 1], float(CAP)), 0.0))
        accs += [jnp.zeros((EL, 128), jnp.float32)] * (64 - CAP - 1)
        acc = jnp.concatenate(accs, axis=0).astype(jnp.bfloat16)
        t = lax.dot_general(jnp.ones((8, 128), jnp.bfloat16), acc, (((1,), (1,)), ((), ())),
                            preferred_element_type=jnp.float32)
        tabv[...] = t.astype(jnp.int32)
        tcp = pltpu.make_async_copy(tabv.at[pl.ds(0, 1)], tab, tsem.at[0])
        tcp.start()
        zrow[...] = jnp.zeros_like(zrow)
        tcp.wait()

        def gather(j):
            if 'g' in abl: return
            def it(s, c):
                tk = jnp.minimum(tab[0, s * EL + j], N - 1)
                pltpu.make_async_copy(x_ref.at[pl.ds(tk, 1)], xg.at[j, pl.ds(s, 1)], xsem.at[j]).start(priority=1 if 'p' in abl else 0)
                return c
            lax.fori_loop(0, CAP, it, 0)

        def send(j):
            if 's' in abl: return
            n = tab[0, CAP * EL + j]
            st = (n * me) >> 2
            cq = (n + 3) >> 2
            def one(s):
                tk = tab[0, s * EL + j]
                pltpu.make_async_remote_copy(
                    ybuf.at[j, pl.ds(s, 1)], stg.at[pl.ds(tk & (ROWS - 1), 1)], ssem.at[j], rsem,
                    device_id=(tk >> 9,), device_id_type=MESH).start()
            @pl.when(n == CAP)
            def _():
                if 'u' in abl:
                    for s in range(CAP):
                        one(s)
                else:
                    def it3(i, c):
                        for k in range(3):
                            one(i * 3 + k)
                        return c
                    lax.fori_loop(0, CAP // 3, it3, 0)
            @pl.when(n < CAP)
            def _():
                def it(s, c):
                    one(s)
                    return c
                lax.fori_loop(0, n, it, 0)

        def wait_send(j, late=False):
            if 'd' in abl and not late: return
            if 's' in abl: return
            n = tab[0, CAP * EL + j]
            def w(sz):
                pltpu.make_async_remote_copy(
                    ybuf.at[j, pl.ds(0, sz)], stg.at[pl.ds(0, sz)], ssem.at[j], rsem,
                    device_id=(me,), device_id_type=MESH).wait_send()
            for bit in (32, 16, 8, 4, 2, 1):
                @pl.when((n & bit) != 0)
                def _():
                    if bit >= 8:
                        w(bit)
                    else:
                        for _k in range(bit):
                            w(1)

        gather(0)
        gather(1)
        fcp.wait()
        def zit(i, c):
            @pl.when(flg[i >> 7, i & 127] == 0)
            def _():
                pltpu.make_async_copy(zrow.at[pl.ds(0, 1)], stg.at[pl.ds(i, 1)], rsem).start()
            return c
        if 's' not in abl and 'z' not in abl: lax.fori_loop(0, ROWS, zit, 0)
        pl.semaphore_wait(bar, ND - 1)

        for j in range(EL):
            for n in (() if 'g' in abl else (48, 1, 1, 1)):
                pltpu.make_async_copy(x_ref.at[pl.ds(0, n)], xg.at[j, pl.ds(0, n)], xsem.at[j]).wait()
            if j==0 or 'n' not in abl: wcp[j].wait()
            if j + inflight < EL and 'n' not in abl:
                wcp[j + inflight].start(priority=1 if 'w' in abl else 0)
            y = jnp.dot(xg[j].astype(jnp.bfloat16), wbuf[j].astype(jnp.bfloat16),
                              preferred_element_type=jnp.float32)
            yb = lax.bitcast_convert_type(y.astype(jnp.bfloat16).astype(jnp.float32), jnp.uint32)
            ybuf[j] = yb[:, :H // 2] | (yb[:, H // 2:] >> 16)
            send(j)
            if j + 2 < EL:
                gather(j + 2)
            if j >= 2:
                wait_send(j - 2)
        if 'd' in abl:
            for j in range(EL): wait_send(j, True)
        wait_send(EL - 2)
        wait_send(EL - 1)
        if 's' not in abl and 'z' not in abl: pltpu.make_async_copy(stg, stg, rsem).wait()
        ocp = []
        for q in range(4):
            r = pl.ds(q * 128, 128)
            v = stg[r, :]
            obuf[r, :H // 2] = lax.bitcast_convert_type(v & jnp.uint32(0xFFFF0000), jnp.float32)
            obuf[r, H // 2:] = lax.bitcast_convert_type(v << 16, jnp.float32)
        for c in ocp:
            c.wait()

    def kernel(x, router_W, route_idx, expert_W):
        del router_W
        idx = route_idx.astype(jnp.int32).reshape(NB, 128)
        hbm = pl.BlockSpec(memory_space=pltpu.HBM)
        return pl.pallas_call(
            body, out_shape=jax.ShapeDtypeStruct((ROWS, H), jnp.float32),
            in_specs=[pl.BlockSpec(memory_space=pltpu.VMEM), hbm, hbm], out_specs=pl.BlockSpec(memory_space=pltpu.VMEM),
            scratch_shapes=[
                pltpu.VMEM((ROWS, H // 2), jnp.uint32),
                pltpu.VMEM((EL, D, H), jnp.float32), pltpu.VMEM((EL, MP, D), jnp.float32),
                pltpu.VMEM((EL, MP, H // 2), jnp.uint32), pltpu.VMEM((NB, E, 128), jnp.float32),
                pltpu.VMEM((8, 512), jnp.int32), pltpu.VMEM((NB, 128), jnp.int32),
                pltpu.VMEM((8, H // 2), jnp.uint32),
                pltpu.SMEM((1, 512), jnp.int32), pltpu.SMEM((4, 128), jnp.int32),
                pltpu.SemaphoreType.DMA((EL,)), pltpu.SemaphoreType.DMA((EL,)), pltpu.SemaphoreType.DMA((EL,)),
                pltpu.SemaphoreType.DMA, pltpu.SemaphoreType.DMA((2,)),
            ],
            compiler_params=pltpu.CompilerParams(collective_id=0, vmem_limit_bytes=48 * 1024 * 1024,
                                                 disable_bounds_checks=nobounds),
        )(idx, x, expert_W)
    return kernel


pallas_dist_moe_cap_ep_outshard_n2048_d512_e8_h1024_kernel = make(8, True, 'wdu')
```
